```python
import numpy as np

kernel_name = "dist_moe_top2_ep_n2048_d512_e4_h1024"

def setup_inputs():
    x = np.random.randn(2048, 512).astype(np.float32)
    router_W = np.random.randn(512, 16).astype(np.float32) * 0.1
    scores64 = x.astype(np.float64) @ router_W.astype(np.float64)
    route_idx = np.argsort(-scores64, axis=-1)[:, :2].astype(np.int32)
    expert_W = np.random.randn(16, 512, 1024).astype(np.float32) * 0.02
    return {"x": x, "router_W": router_W, "route_idx": route_idx, "expert_W": expert_W}

def reference(x, router_W, route_idx, expert_W):
    scores = x @ router_W
    s_max = scores.max(axis=-1, keepdims=True)
    probs = np.exp(scores - s_max)
    probs = probs / probs.sum(axis=-1, keepdims=True)
    out = np.zeros((2048, 1024), dtype=np.float32)
    for i in range(2048):
        e0, e1 = int(route_idx[i, 0]), int(route_idx[i, 1])
        g0, g1 = probs[i, e0], probs[i, e1]
        gs = g0 + g1
        out[i] = (g0 / gs) * (x[i] @ expert_W[e0]) + (g1 / gs) * (x[i] @ expert_W[e1])
    return out
```

```python
import contextlib

import jax
import jax.numpy as jnp
from jax import lax
from jax.experimental import pallas as pl
from jax.experimental.pallas import tpu as pltpu

N, D, H = 2048, 512, 1024
NDEV = 4
EL = 4
NE = NDEV * EL
BS = 128
NB = N // BS
CAP = BS // NDEV
SEG = N // NDEV
HALF = SEG // 2
QUART = SEG // 4
WC = 128
NC = H // WC
GB = 4
NG = NB // GB
GT = GB * BS
WIN = 40
SELR = CAP + 3 * WIN
XST = 512
XMAX = 3 * SEG
XROWS = XMAX + 128
ZST = 640
NBIT = 6

F32 = jnp.float32
BF16 = jnp.bfloat16
I32 = jnp.int32
MESH = pl.DeviceIdType.MESH

PROFILE = False


def _scope(name):
    return jax.named_scope(name) if PROFILE else contextlib.nullcontext()


class _Marker:
    def __init__(self):
        self.cur = None

    def __call__(self, name):
        if self.cur is not None:
            self.cur.__exit__(None, None, None)
            self.cur = None
        if name is not None:
            self.cur = _scope(name)
            self.cur.__enter__()


def _iota(shape, dim):
    return lax.broadcasted_iota(I32, shape, dim)


def _onehot(mask):
    return jnp.where(mask, 1.0, 0.0).astype(BF16)


def _pad16(n):
    return (n + 15) & (-16)


def _dot(a, b):
    return jnp.dot(a, b, preferred_element_type=F32)


def _dot_nt(a, b):
    return lax.dot_general(a, b, (((1,), (1,)), ((), ())),
                           preferred_element_type=F32)


def _kernel(x_hbm, wr_hbm, r_hbm, w_hbm, out_ref,
            xf, xb, wrf, rv, wf, wb,
            codes, pcol, tabv, tabs,
            xe_f, me_f, xe_b, xo_b, mo_f,
            yexp, recv, yown, s0, s1, pm, ag,
            sem_in, sem_send, sem_p1, sem_ag):
    mark = _Marker()
    mark("issue")
    me = lax.axis_index("i")
    right = (me + 1) & 3
    diag_dev = (me + 2) & 3
    left = (me + 3) & 3
    peers = (diag_dev, right, left)

    def x_copy(g):
        rows = pl.ds(pl.multiple_of(g * GT, GT), GT)
        return pltpu.make_async_copy(x_hbm.at[rows], xf.at[rows], sem_in.at[3 + g])

    def w_copy(h, e):
        cols = pl.ds(pl.multiple_of(h * WC, WC), WC)
        return pltpu.make_async_copy(w_hbm.at[e, :, cols], wf.at[h, e],
                                     sem_in.at[3 + NG + h * EL + e])

    r_copy = pltpu.make_async_copy(r_hbm, rv, sem_in.at[0])
    wr_copy = pltpu.make_async_copy(wr_hbm, wrf, sem_in.at[1])
    r_copy.start()
    wr_copy.start()
    for g in range(NG):
        x_copy(g).start()
    for h in range(NC):
        for e in range(EL):
            w_copy(h, e).start()

    barrier = pltpu.get_barrier_semaphore()
    for dev in peers:
        pl.semaphore_signal(barrier, 1, device_id=(dev,), device_id_type=MESH)

    mark("zero")
    xe_f[0:ZST, :] = jnp.zeros((ZST, D), F32)
    me_f[0:ZST, :] = jnp.zeros((ZST, 128), F32)

    mark("rwait")
    r_copy.wait()
    mark("meta")
    e0 = rv[pl.ds(0, NB, stride=2), :]
    e1 = rv[pl.ds(1, NB, stride=2), :]
    c0 = e0 >> 2
    c1 = e1 >> 2
    lane = _iota((NB, BS), 1)
    z = _iota((NB, BS), 0) & 3
    c0z = c0 ^ z
    c1z = c1 ^ z
    is_diag = (c0 ^ c1) == 2
    fixed = jnp.logical_not(is_diag)
    pref = jnp.where((lane & 1) == 0, c0z, c1z)
    masks_a = [fixed & (pref == o) for o in range(NDEV)]
    masks_a += [is_diag & ((c0z & 1) == 0), is_diag & ((c0z & 1) == 1)]
    i0 = _iota((BS, BS), 0)
    i1 = _iota((BS, BS), 1)
    uo = jnp.concatenate([_onehot(i0 < i1), jnp.ones((BS, BS), BF16)], axis=1)

    def stack(ms):
        return jnp.concatenate([jnp.where(m, 1.0, 0.0) for m in ms], axis=0).astype(BF16)

    def part(a, k):
        return a[NB * k:NB * (k + 1), :]

    ra = _dot(stack(masks_a), uo).astype(I32)
    rank_a, tot_a = ra[:, :BS], ra[:, BS:]
    load = [part(tot_a, o) for o in range(NDEV)]
    rank_f = sum(jnp.where(masks_a[o], part(rank_a, o), 0) for o in range(NDEV))
    over = [jnp.maximum(load[o] - CAP, 0) for o in range(NDEV)]
    ovbase = [0, over[0], over[0] + over[1], over[0] + over[1] + over[2]]
    ovb = sum(jnp.where(masks_a[o], ovbase[o], 0) for o in range(1, NDEV))
    tot02, tot13 = part(tot_a, 4), part(tot_a, 5)
    jf = jnp.where(masks_a[4], part(rank_a, 4),
                   jnp.where(masks_a[5], tot02 + part(rank_a, 5),
                             tot02 + tot13 + ovb + rank_f - CAP))
    flex = is_diag | (rank_f >= CAP)
    used = [jnp.minimum(load[o], CAP) for o in range(NDEV)]
    g2 = CAP - used[0]
    g1 = g2 + CAP - used[2]
    g3 = g1 + CAP - used[1]
    p_flex = jnp.where(
        jf < g2, used[0] + jf,
        jnp.where(jf < g1, 2 * CAP + used[2] + jf - g2,
                  jnp.where(jf < g3, CAP + used[1] + jf - g1,
                            3 * CAP + used[3] + jf - g3)))
    p = jnp.where(flex, p_flex, pref * CAP + rank_f) ^ (z << 5)
    owner = p >> 5

    def inv(s):
        return (c0 == s) | (c1 == s)

    masks_b = [inv(me) & (owner == o) for o in peers]
    masks_b += [inv(s) & (owner == me) for s in peers]
    masks_b += [inv(left) & (owner == right), inv(diag_dev) & (owner == right),
                inv(right) & (owner == left)]
    nmb = len(masks_b)
    rb = _dot(stack(masks_b), uo)
    rank_b = rb[:, :BS].astype(I32)
    tot_b = rb[:, BS:].astype(BF16)
    j0 = _iota((NB * nmb + NB, NB * nmb), 0)
    j1 = _iota((NB * nmb + NB, NB * nmb), 1)
    pre = (((j0 >> 4) == (j1 >> 4)) & (j1 < j0)
           | ((j0 - NB * nmb) == (j1 >> 4)) & (j0 >= NB * nmb))
    cb = _dot(_onehot(pre), tot_b).astype(I32)
    cum_b, n_b = cb[:NB * nmb, :], cb[NB * nmb:, :]
    n16 = _pad16(n_b)
    xoff = [0, n16[0:1, :], n16[0:1, :] + n16[1:2, :]]
    roff = [0, n16[3:4, :], n16[3:4, :] + n16[4:5, :]]

    codes[0] = e0
    codes[1] = e1
    codes[2] = jnp.where(owner == me, p & (CAP - 1), -1)
    for k in range(3):
        codes[3 + k] = jnp.where(
            masks_b[k], part(rank_b, k) + ((xoff[k] + part(cum_b, k)) & 7), -1)
        ic = jnp.where(masks_b[3 + k],
                       roff[k] + part(cum_b, 3 + k) + part(rank_b, 3 + k) + 1, 0)
        codes[6 + k] = ic & (-32)
        codes[9 + k] = ic & 31

    def diag_row(v):
        r = v.shape[0]
        sel = _iota((r, BS), 0) == _iota((r, BS), 1)
        return jnp.sum(jnp.where(sel, v, 0).astype(F32), axis=0, keepdims=True).astype(I32)

    tabv[...] = jnp.concatenate(
        [diag_row(cum_b[:3 * NB, :]), diag_row(n_b), jnp.zeros((6, BS), I32)], axis=0)
    tab_copy = pltpu.make_async_copy(tabv, tabs, sem_in.at[2])
    tab_copy.start()

    pcol[...] = jnp.concatenate(
        [p.astype(F32), jnp.zeros((BS - NB, BS), F32)], axis=0).T

    wr_copy.wait()
    wr = wrf[...]
    wr_hi = wr.astype(BF16)
    wr_lo = (wr - wr_hi.astype(F32)).astype(BF16)
    wr2 = jnp.concatenate([wr_hi, wr_lo], axis=0)

    mark("tabwait")
    tab_copy.wait()
    mark("zero2")
    n_out = [tabs[1, k] for k in range(3)]
    n_in = [tabs[1, 3 + k] for k in range(3)]
    xo = [0, _pad16(n_out[0]), _pad16(n_out[0]) + _pad16(n_out[1])]
    xtot = xo[2] + _pad16(n_out[2])
    ro = [0, _pad16(n_in[0]), _pad16(n_in[0]) + _pad16(n_in[1])]
    ktot = ro[2] + _pad16(n_in[2])
    do = [0, _pad16(tabs[1, 6]) + _pad16(tabs[1, 7]), _pad16(tabs[1, 8])]
    xtiles = (xtot + 127) >> 7
    ktiles = (ktot + 127) >> 7

    def zero_tile(j, c):
        rows = pl.ds(pl.multiple_of(j * 128, 128), 128)
        xe_f[rows, :] = jnp.zeros((128, D), F32)
        me_f[rows, :] = jnp.zeros((128, 128), F32)
        return c

    lax.fori_loop(ZST // 128, (xtot + WIN + 127) >> 7, zero_tile, 0)
    mark(None)

    tgt = jnp.concatenate(
        [_iota((CAP, BS), 0)] + [_iota((WIN, BS), 0)] * 3, axis=0)
    erow = _iota((NE, BS), 0)

    def smat(meta, base, width):
        col = _iota((meta.shape[0], width), 1) + (base + 1)
        ics = [meta[:, 4 + k:5 + k].astype(I32) for k in range(3)]
        return _onehot((col == ics[0]) | (col == ics[1]) | (col == ics[2]))

    def group(g, c):
        with _scope("xwait"):
            x_copy(g).wait()
        gm_ = _Marker()
        gm_("group")
        rows = pl.ds(pl.multiple_of(g * GT, GT), GT)
        xb[...] = xf[rows, :].astype(BF16)
        sc2 = _dot_nt(wr2, xb[...])
        sc = sc2[:NE, :] + sc2[NE:, :]
        for j in range(GB):
            a = g * GB + j

            def code(k):
                return codes[k, pl.ds(a, 1), :]

            s = sc[:, j * BS:(j + 1) * BS]
            ex = jnp.exp(s - jnp.max(s, axis=0, keepdims=True))
            pr = ex / jnp.sum(ex, axis=0, keepdims=True)
            ea, eb = code(0), code(1)
            ga = jnp.sum(jnp.where(erow == ea, pr, 0.0), axis=0, keepdims=True)
            gb = jnp.sum(jnp.where(erow == eb, pr, 0.0), axis=0, keepdims=True)
            gs = ga + gb
            wa, wb_ = ga / gs, gb / gs
            hi, lo = [], []
            for e in range(EL):
                ge = me * EL + e
                m = jnp.where(ea == ge, wa, 0.0) + jnp.where(eb == ge, wb_, 0.0)
                mh = m.astype(BF16).astype(F32)
                hi.append(mh)
                lo.append(m - mh)
            hi += [code(6 + k).astype(F32) for k in range(3)] + [jnp.zeros((1, BS), F32)]
            lo += [code(9 + k).astype(F32) for k in range(3)] + [jnp.zeros((1, BS), F32)]
            meta = jnp.concatenate(hi + lo, axis=0).astype(BF16)

            cd = jnp.concatenate(
                [jnp.broadcast_to(code(2), (CAP, BS))]
                + [jnp.broadcast_to(code(3 + k), (WIN, BS)) for k in range(3)], axis=0)
            sel = _onehot(cd == tgt)
            gx = _dot(sel, xb[j * BS:(j + 1) * BS, :])
            gm2 = _dot_nt(sel, meta)
            gm = gm2[:, :8] + gm2[:, 8:]
            orow = pl.ds(pl.multiple_of(a * CAP, CAP), CAP)
            xo_b[orow, :] = gx[:CAP].astype(BF16)
            mo_f[orow, 0:8] = gm[:CAP]
            s0[orow, :] = smat(gm[:CAP], 0, XST)
            for k in range(3):
                st = pl.multiple_of((xo[k] + tabs[0, k * NB + a]) & (-8), 8)
                wrow = pl.ds(st, WIN)
                lo_ = CAP + k * WIN
                xe_f[wrow, :] += gx[lo_:lo_ + WIN]
                me_f[wrow, 0:8] += gm[lo_:lo_ + WIN]
        gm_(None)
        return c

    lax.fori_loop(0, NG, group, 0)

    def finalize(rows):
        xe_b[rows, :] = xe_f[rows, :].astype(BF16)

    mark("finalize")
    finalize(pl.ds(0, XST))

    def finalize_tile(j, c):
        finalize(pl.ds(pl.multiple_of(j * 128, 128), 128))
        return c

    lax.fori_loop(XST // 128, xtiles, finalize_tile, 0)
    mark(None)

    def remote(h, src, dst, rsem, dev):
        return pltpu.make_async_remote_copy(
            src_ref=src, dst_ref=dst, send_sem=sem_send.at[h], recv_sem=rsem,
            device_id=(dev,), device_id_type=MESH)

    def pieces(n_rows, fn):
        u = (n_rows + 15) >> 4
        for bit in reversed(range(NBIT)):
            @pl.when(((u >> bit) & 1) == 1)
            def _(bit=bit):
                off = ((u >> (bit + 1)) << (bit + 1)) * 16
                fn(bit, off, 16 << bit)

    def p1_desc(h, k, bit, off, size):
        src = yexp.at[h, pl.ds(pl.multiple_of(xo[k] + off, 16), size)]
        dst = recv.at[h, pl.ds(pl.multiple_of(do[k] + off, 16), size)]
        slot = (0, 2, 1)[k]
        return remote(h, src, dst, sem_p1.at[h, slot, bit], peers[k])

    def expert_rows(xv, meta, h, before=None):
        acc = None
        for e in range(EL):
            if before is not None:
                before(e)
            r = _dot(xv, wb[h, e]) * meta[:, e:e + 1]
            acc = r if acc is None else acc + r
        return acc

    def load_w(h, es):
        for e in es:
            w_copy(h, e).wait()
        for e in es:
            wb[h, e] = wf[h, e].astype(BF16)

    def exports(h, fine=False):
        m_ = _Marker()
        m_("exports")
        if not fine:
            load_w(h, range(EL))
        yexp[h, 0:XST, :] = expert_rows(
            xe_b[0:XST, :], me_f[0:XST, 0:8], h,
            (lambda e: load_w(h, (e, e + 1)) if e % 2 == 0 else None) if fine else None
        ).astype(BF16)

        def tile(j, c):
            rows = pl.ds(pl.multiple_of(j * 128, 128), 128)
            yexp[h, rows, :] = expert_rows(xe_b[rows, :], me_f[rows, 0:8], h).astype(BF16)
            return c

        lax.fori_loop(XST // 128, xtiles, tile, 0)
        m_("p1send")
        for k in range(3):
            pieces(n_out[k], lambda bit, off, size, k=k: p1_desc(h, k, bit, off, size).start())
        m_(None)

    def own(h):
        yown[...] = expert_rows(xo_b[...], mo_f[:, 0:8], h)

    def p1_wait(h):
        for k in range(3):
            def w(bit, off, size, k=k):
                dst = recv.at[h, pl.ds(pl.multiple_of(ro[k] + off, 16), size)]
                remote(h, dst, dst, sem_p1.at[h, k, bit], me).wait_recv()
            pieces(n_in[k], w)

    def seg(h, o, half):
        return ag.at[h, pl.ds(pl.multiple_of(o * SEG + half * HALF, HALF), HALF)]

    def quarter(h, o, q):
        return ag.at[h, pl.ds(pl.multiple_of(o * SEG + q * QUART, QUART), QUART)]

    def combine(h):
        rv_ = jnp.where(_iota((XST, WC), 0) < ktot, recv[h, 0:XST, :], jnp.zeros((), BF16))
        yown[...] += _dot(s0[...], rv_)

        def tile(j, c):
            rows = pl.ds(pl.multiple_of(j * 128, 128), 128)
            valid = (_iota((128, WC), 0) + j * 128) < ktot
            t = jnp.where(valid, recv[h, rows, :], jnp.zeros((), BF16))
            yown[...] += _dot(s1[j - XST // 128], t)
            return c

        lax.fori_loop(XST // 128, ktiles, tile, 0)
        ag[h, pl.ds(pl.multiple_of(me * SEG, SEG), SEG), :] = yown[...].astype(BF16)

    def ag_send(h):
        for dev, half, k in ((right, 0, 0), (left, 1, 2), (right, 1, 1), (left, 0, 3)):
            remote(h, seg(h, me, half), seg(h, me, half), sem_ag.at[h, k], dev).start()

    def forward(h):
        for src_dev, half, k, dev, kf in ((left, 0, 0, right, 4), (right, 1, 2, left, 6)):
            s_ = seg(h, src_dev, half)
            remote(h, s_, s_, sem_ag.at[h, k], me).wait_recv()
            for j in range(2):
                q_ = quarter(h, src_dev, 2 * half + j)
                remote(h, q_, q_, sem_ag.at[h, kf + j], dev).start()

    def unperm(h, blocks):
        cols = pl.ds(pl.multiple_of(h * WC, WC), WC)
        for b in blocks:
            rhs = jnp.concatenate(
                [ag[h, o * SEG + b * CAP:o * SEG + (b + 1) * CAP, :] for o in range(NDEV)],
                axis=0)
            out_ref[b * BS:(b + 1) * BS, cols] = _dot(pm[b], rhs)

    def finish(h):
        with _scope("finwait"):
            for src_dev, half, k in ((left, 1, 1), (right, 0, 3)):
                s_ = seg(h, src_dev, half)
                remote(h, s_, s_, sem_ag.at[h, k], me).wait_recv()
        for j in range(2):
            with _scope("finwait"):
                for half in range(2):
                    q_ = quarter(h, diag_dev, 2 * half + j)
                    remote(h, q_, q_, sem_ag.at[h, 4 + 2 * half + j], me).wait_recv()
            with _scope("unperm"):
                unperm(h, [8 * half + 4 * j + b for half in range(2) for b in range(4)])

    def wait_sends(h):
        for k in range(3):
            pieces(n_out[k], lambda bit, off, size, k=k: p1_desc(h, k, bit, off, size).wait_send())
        for _ in range(6):
            s_ = seg(h, me, 0)
            remote(h, s_, s_, sem_ag.at[h, 0], me).wait_send()

    def middle(h):
        with _scope("own"):
            own(h)
        with _scope("p1wait"):
            p1_wait(h)
        with _scope("combine"):
            combine(h)
        with _scope("agsend"):
            ag_send(h)

    def late_setup():
        def tile(j, c):
            s1[j - XST // 128] = smat(mo_f[:, 0:8], j * 128, 128)
            return c

        lax.fori_loop(XST // 128, ktiles, tile, 0)

    def unperm_setup():
        pc = pcol[...].astype(I32)
        for b in range(NB):
            pm[b] = _onehot(pc[:, b:b + 1] == i1)

    late_setup()
    with _scope("barrier"):
        pl.semaphore_wait(barrier, 3)

    def step(i, c):
        @pl.when(i + 3 < NC)
        def _():
            exports(i + 3)

        @pl.when((i >= -1) & (i + 1 < NC))
        def _():
            middle(i + 1)

        @pl.when(i == -1)
        def _():
            with _scope("unperm_setup"):
                unperm_setup()

        @pl.when((i >= 0) & (i < NC))
        def _():
            with _scope("forward"):
                forward(i)

        @pl.when(i >= 1)
        def _():
            finish(i - 1)

        @pl.when(i >= 2)
        def _():
            with _scope("sendwait"):
                wait_sends(i - 2)

        return c

    lax.fori_loop(-3, NC + 1, step, 0)
    with _scope("drain"):
        wait_sends(NC - 1)


def pallas_dist_moe_top2_ep_n2048_d512_e4_h1024_kernel(
    x: jax.Array,
    router_W: jax.Array,
    route_idx: jax.Array,
    expert_W: jax.Array,
):
    wr_t = router_W.T
    r32 = route_idx.astype(I32).T.reshape(2, NB, BS).transpose(1, 0, 2).reshape(2 * NB, BS)

    any_spec = pl.BlockSpec(memory_space=pl.ANY)
    vmem = pltpu.VMEM
    scratch = [
        vmem((N, D), F32),
        vmem((GT, D), BF16),
        vmem((NE, D), F32),
        vmem((2 * NB, BS), I32),
        vmem((NC, EL, D, WC), F32),
        vmem((NC, EL, D, WC), BF16),
        vmem((12, NB, BS), I32),
        vmem((BS, BS), F32),
        vmem((8, BS), I32),
        pltpu.SMEM((8, BS), I32),
        vmem((XROWS, D), F32),
        vmem((XROWS, 128), F32),
        vmem((XMAX, D), BF16),
        vmem((SEG, D), BF16),
        vmem((SEG, 128), F32),
        vmem((NC, XMAX, WC), BF16),
        vmem((NC, XMAX, WC), BF16),
        vmem((SEG, WC), F32),
        vmem((SEG, XST), BF16),
        vmem(((XMAX - XST) // 128, SEG, 128), BF16),
        vmem((NB, BS, BS), BF16),
        vmem((NC, N, WC), BF16),
        pltpu.SemaphoreType.DMA((3 + NG + NC * EL,)),
        pltpu.SemaphoreType.DMA((NC,)),
        pltpu.SemaphoreType.DMA((NC, 3, NBIT)),
        pltpu.SemaphoreType.DMA((NC, 8)),
    ]
    return pl.pallas_call(
        _kernel,
        out_shape=pltpu.VMEM((N, H), F32),
        in_specs=[any_spec] * 4,
        out_specs=pl.BlockSpec(memory_space=pltpu.VMEM),
        scratch_shapes=scratch,
        compiler_params=pltpu.CompilerParams(
            collective_id=0, vmem_limit_bytes=100 * 1024 * 1024,
            disable_semaphore_checks=True, disable_bounds_checks=True),
    )(x, wr_t, r32, expert_W)
```

```python
import jax
import jax.numpy as jnp
from jax import lax
from jax.experimental import pallas as pl
from jax.experimental.pallas import tpu as pltpu

N, D, H = 2048, 512, 1024
NDEV = 4
EL = 4
NE = NDEV * EL
BS = 128
NB = N // BS
CAP = BS // NDEV
SEG = N // NDEV
HALF = SEG // 2
QUART = SEG // 4
WC = 128
NC = H // WC
GB = 2
NG = NB // GB
GT = GB * BS
WIN = 40
SELR = CAP + 3 * WIN
XST = 512
XMAX = 3 * SEG
XROWS = XMAX + 128
ZST = 640
NBIT = 6

F32 = jnp.float32
BF16 = jnp.bfloat16
I32 = jnp.int32
MESH = pl.DeviceIdType.MESH


def _iota(shape, dim):
    return lax.broadcasted_iota(I32, shape, dim)


def _onehot(mask):
    return jnp.where(mask, 1.0, 0.0).astype(BF16)


def _pad16(n):
    return (n + 15) & (-16)


def _dot(a, b):
    return jnp.dot(a, b, preferred_element_type=F32)


def _dot_nt(a, b):
    return lax.dot_general(a, b, (((1,), (1,)), ((), ())),
                           preferred_element_type=F32)


def _kernel(x_hbm, wr_hbm, r_hbm, w_hbm, out_ref,
            xf, xb, wrf, rv, wf, wb,
            codes, pcol, tabv, tabs,
            xe_f, me_f, xe_b, xo_b, mo_f,
            yexp, recv, yown, s0, s1, pm, ag,
            sem_in, sem_send, sem_p1, sem_ag):
    me = lax.axis_index("i")
    right = (me + 1) & 3
    diag = (me + 2) & 3
    left = (me + 3) & 3
    peers = (diag, right, left)

    def x_copy(g):
        rows = pl.ds(pl.multiple_of(g * GT, GT), GT)
        return pltpu.make_async_copy(x_hbm.at[rows], xf.at[rows], sem_in.at[3 + g])

    def w_copy(h, e):
        cols = pl.ds(pl.multiple_of(h * WC, WC), WC)
        return pltpu.make_async_copy(w_hbm.at[e, :, cols], wf.at[h, e],
                                     sem_in.at[3 + NG + h * EL + e])

    r_copy = pltpu.make_async_copy(r_hbm, rv, sem_in.at[0])
    wr_copy = pltpu.make_async_copy(wr_hbm, wrf, sem_in.at[1])
    r_copy.start()
    wr_copy.start()
    for g in range(NG):
        x_copy(g).start()
    for h in range(NC):
        for e in range(EL):
            w_copy(h, e).start()

    barrier = pltpu.get_barrier_semaphore()
    for dev in peers:
        pl.semaphore_signal(barrier, 1, device_id=(dev,), device_id_type=MESH)

    xe_f[0:ZST, :] = jnp.zeros((ZST, D), F32)
    me_f[0:ZST, :] = jnp.zeros((ZST, 128), F32)

    r_copy.wait()
    e0 = rv[pl.ds(0, NB, stride=2), :]
    e1 = rv[pl.ds(1, NB, stride=2), :]
    c0 = e0 >> 2
    c1 = e1 >> 2
    i0 = _iota((BS, BS), 0)
    i1 = _iota((BS, BS), 1)
    upper = _onehot(i0 < i1)
    uo = jnp.concatenate([upper, jnp.ones((BS, BS), BF16)], axis=1)

    def stack(ms):
        return jnp.concatenate([jnp.where(m, 1.0, 0.0) for m in ms], axis=0).astype(BF16)

    def part(a, k):
        return a[NB * k:NB * (k + 1), :]

    is_diag = (c0 ^ c1) == 2
    fixed = jnp.logical_not(is_diag)
    adj = fixed & (c0 != c1)
    low = jnp.where(((c1 - c0) & 3) == 1, c0, c1)
    masks_c = [adj & (low == a) for a in range(NDEV)]
    rc = _dot(stack(masks_c), upper).astype(I32)
    rank_c = sum(jnp.where(masks_c[a], part(rc, a), 0) for a in range(NDEV))
    flip = (rank_c + _iota((NB, BS), 0)) & 1
    pref = jnp.where(adj, (low + flip) & 3, c0)
    masks_a = [fixed & (pref == o) for o in range(NDEV)]
    masks_a += [is_diag & ((c0 & 1) == 0), is_diag & ((c0 & 1) == 1)]
    ra = _dot(stack(masks_a), uo).astype(I32)
    rank_a, tot_a = ra[:, :BS], ra[:, BS:]
    load = [part(tot_a, o) for o in range(NDEV)]
    rank_f = sum(jnp.where(masks_a[o], part(rank_a, o), 0) for o in range(NDEV))
    over = [jnp.maximum(load[o] - CAP, 0) for o in range(NDEV)]
    ovbase = [0, over[0], over[0] + over[1], over[0] + over[1] + over[2]]
    ovb = sum(jnp.where(masks_a[o], ovbase[o], 0) for o in range(1, NDEV))
    tot02, tot13 = part(tot_a, 4), part(tot_a, 5)
    jf = jnp.where(masks_a[4], part(rank_a, 4),
                   jnp.where(masks_a[5], tot02 + part(rank_a, 5),
                             tot02 + tot13 + ovb + rank_f - CAP))
    flex = is_diag | (rank_f >= CAP)
    used = [jnp.minimum(load[o], CAP) for o in range(NDEV)]
    g2 = CAP - used[0]
    g1 = g2 + CAP - used[2]
    g3 = g1 + CAP - used[1]
    p_flex = jnp.where(
        jf < g2, used[0] + jf,
        jnp.where(jf < g1, 2 * CAP + used[2] + jf - g2,
                  jnp.where(jf < g3, CAP + used[1] + jf - g1,
                            3 * CAP + used[3] + jf - g3)))
    p = jnp.where(flex, p_flex, pref * CAP + rank_f)
    owner = p >> 5

    def involves(s):
        return (c0 == s) | (c1 == s)

    masks_b = [involves(me) & (owner == o) for o in peers]
    masks_b += [involves(s) & (owner == me) for s in peers]
    masks_b += [involves(left) & (owner == right), involves(diag) & (owner == right),
                involves(right) & (owner == left)]
    nrow = NB * len(masks_b)
    rb = _dot(stack(masks_b), uo)
    rank_b = rb[:, :BS].astype(I32)
    tot_b = rb[:, BS:].astype(BF16)
    j0 = _iota((nrow + NB, nrow), 0)
    j1 = _iota((nrow + NB, nrow), 1)
    pre = ((((j0 >> 4) == (j1 >> 4)) & (j1 < j0))
           | (((j0 - nrow) == (j1 >> 4)) & (j0 >= nrow)))
    cb = _dot(_onehot(pre), tot_b).astype(I32)
    cum_b, n_b = cb[:nrow, :], cb[nrow:, :]
    n16 = _pad16(n_b)
    xoff = [0, n16[0:1, :], n16[0:1, :] + n16[1:2, :]]
    roff = [0, n16[3:4, :], n16[3:4, :] + n16[4:5, :]]

    codes[0] = e0
    codes[1] = e1
    codes[2] = jnp.where(owner == me, p & (CAP - 1), -1)
    starts = []
    for k in range(3):
        start = xoff[k] + part(cum_b, k)
        starts.append(start & (-8))
        codes[3 + k] = jnp.where(masks_b[k], part(rank_b, k) + (start & 7), -1)
        ic = jnp.where(masks_b[3 + k],
                       roff[k] + part(cum_b, 3 + k) + part(rank_b, 3 + k) + 1, 0)
        codes[6 + k] = ic & (-32)
        codes[9 + k] = ic & 31

    def diag_row(v):
        sel = _iota(v.shape, 0) == _iota(v.shape, 1)
        return jnp.sum(jnp.where(sel, v, 0).astype(F32), axis=0, keepdims=True).astype(I32)

    tabv[...] = jnp.concatenate(
        [diag_row(jnp.concatenate(starts, axis=0)), diag_row(n_b), jnp.zeros((6, BS), I32)],
        axis=0)
    tab_copy = pltpu.make_async_copy(tabv, tabs, sem_in.at[2])
    tab_copy.start()

    pcol[...] = jnp.concatenate(
        [p.astype(F32), jnp.zeros((BS - NB, BS), F32)], axis=0).T

    wr_copy.wait()
    wr = wrf[...]
    wr_hi = wr.astype(BF16)
    wr_lo = (wr - wr_hi.astype(F32)).astype(BF16)
    wr2 = jnp.concatenate([wr_hi, wr_lo], axis=0)

    tab_copy.wait()
    n_out = [tabs[1, k] for k in range(3)]
    n_in = [tabs[1, 3 + k] for k in range(3)]
    xo = [0, _pad16(n_out[0]), _pad16(n_out[0]) + _pad16(n_out[1])]
    xtot = xo[2] + _pad16(n_out[2])
    ro = [0, _pad16(n_in[0]), _pad16(n_in[0]) + _pad16(n_in[1])]
    ktot = ro[2] + _pad16(n_in[2])
    do = [0, _pad16(tabs[1, 6]) + _pad16(tabs[1, 7]), _pad16(tabs[1, 8])]
    xtiles = (xtot + 127) >> 7
    ktiles = (ktot + 127) >> 7

    def tile_rows(j):
        return pl.ds(pl.multiple_of(j * 128, 128), 128)

    def zero_tile(j, c):
        xe_f[tile_rows(j), :] = jnp.zeros((128, D), F32)
        me_f[tile_rows(j), :] = jnp.zeros((128, 128), F32)
        return c

    lax.fori_loop(ZST // 128, (xtot + WIN + 127) >> 7, zero_tile, 0)

    tgt = jnp.concatenate(
        [_iota((CAP, BS), 0)] + [_iota((WIN, BS), 0)] * 3, axis=0)
    erow = _iota((NE, BS), 0)

    def smat(meta, base, width):
        col = _iota((meta.shape[0], width), 1) + (base + 1)
        ics = [meta[:, 4 + k:5 + k].astype(I32) for k in range(3)]
        return _onehot((col == ics[0]) | (col == ics[1]) | (col == ics[2]))

    def group(g, c):
        x_copy(g).wait()
        xb[...] = xf[pl.ds(pl.multiple_of(g * GT, GT), GT), :].astype(BF16)
        sc2 = _dot_nt(wr2, xb[...])
        sc = sc2[:NE, :] + sc2[NE:, :]
        for j in range(GB):
            a = g * GB + j

            def code(k):
                return codes[k, pl.ds(a, 1), :]

            s = sc[:, j * BS:(j + 1) * BS]
            ex = jnp.exp(s - jnp.max(s, axis=0, keepdims=True))
            pr = ex / jnp.sum(ex, axis=0, keepdims=True)
            ea, eb = code(0), code(1)
            ga = jnp.sum(jnp.where(erow == ea, pr, 0.0), axis=0, keepdims=True)
            gb = jnp.sum(jnp.where(erow == eb, pr, 0.0), axis=0, keepdims=True)
            gs = ga + gb
            wa, wb_ = ga / gs, gb / gs
            hi, lo = [], []
            for e in range(EL):
                ge = me * EL + e
                m = jnp.where(ea == ge, wa, 0.0) + jnp.where(eb == ge, wb_, 0.0)
                mh = m.astype(BF16).astype(F32)
                hi.append(mh)
                lo.append(m - mh)
            hi += [code(6 + k).astype(F32) for k in range(3)] + [jnp.zeros((1, BS), F32)]
            lo += [code(9 + k).astype(F32) for k in range(3)] + [jnp.zeros((1, BS), F32)]
            meta = jnp.concatenate(hi + lo, axis=0).astype(BF16)

            cd = jnp.concatenate(
                [jnp.broadcast_to(code(2), (CAP, BS))]
                + [jnp.broadcast_to(code(3 + k), (WIN, BS)) for k in range(3)], axis=0)
            sel = _onehot(cd == tgt)
            gx = _dot(sel, xb[j * BS:(j + 1) * BS, :])
            gm2 = _dot_nt(sel, meta)
            gm = gm2[:, :8] + gm2[:, 8:]
            orow = pl.ds(pl.multiple_of(a * CAP, CAP), CAP)
            xo_b[orow, :] = gx[:CAP].astype(BF16)
            mo_f[orow, 0:8] = gm[:CAP]
            s0[orow, :] = smat(gm[:CAP], 0, XST)
            for k in range(3):
                wrow = pl.ds(pl.multiple_of(tabs[0, k * NB + a], 8), WIN)
                lo_ = CAP + k * WIN
                xe_f[wrow, :] += gx[lo_:lo_ + WIN]
                me_f[wrow, 0:8] += gm[lo_:lo_ + WIN]
        return c

    lax.fori_loop(0, NG, group, 0)

    xe_b[0:XST, :] = xe_f[0:XST, :].astype(BF16)

    def extra_tile_setup(j, c):
        xe_b[tile_rows(j), :] = xe_f[tile_rows(j), :].astype(BF16)
        return c

    def extra_smat(j, c):
        s1[j - XST // 128] = smat(mo_f[:, 0:8], j * 128, 128)
        return c

    lax.fori_loop(XST // 128, xtiles, extra_tile_setup, 0)
    lax.fori_loop(XST // 128, ktiles, extra_smat, 0)

    def remote(h, src, dst, rsem, dev):
        return pltpu.make_async_remote_copy(
            src_ref=src, dst_ref=dst, send_sem=sem_send.at[h], recv_sem=rsem,
            device_id=(dev,), device_id_type=MESH)

    def pieces(n_rows, fn):
        u = (n_rows + 15) >> 4
        for bit in reversed(range(NBIT)):
            @pl.when(((u >> bit) & 1) == 1)
            def _(bit=bit):
                fn(bit, ((u >> (bit + 1)) << (bit + 1)) * 16, 16 << bit)

    def p1_copy(h, k, bit, off, size):
        src = yexp.at[h, pl.ds(pl.multiple_of(xo[k] + off, 16), size)]
        dst = recv.at[h, pl.ds(pl.multiple_of(do[k] + off, 16), size)]
        slot = (0, 2, 1)[k]
        return remote(h, src, dst, sem_p1.at[h, slot, bit], peers[k])

    def expert_rows(xv, meta, h, before=None):
        acc = None
        for e in range(EL):
            if before is not None:
                before(e)
            r = _dot(xv, wb[h, e]) * meta[:, e:e + 1]
            acc = r if acc is None else acc + r
        return acc

    def load_w(h, es):
        for e in es:
            w_copy(h, e).wait()
        for e in es:
            wb[h, e] = wf[h, e].astype(BF16)

    def exports(h, as_weights_arrive=False):
        before = None
        if as_weights_arrive:
            def before(e):
                if e % 2 == 0:
                    load_w(h, (e, e + 1))
        else:
            load_w(h, range(EL))
        yexp[h, 0:XST, :] = expert_rows(
            xe_b[0:XST, :], me_f[0:XST, 0:8], h, before).astype(BF16)

        def tile(j, c):
            rows = tile_rows(j)
            yexp[h, rows, :] = expert_rows(xe_b[rows, :], me_f[rows, 0:8], h).astype(BF16)
            return c

        lax.fori_loop(XST // 128, xtiles, tile, 0)
        for k in range(3):
            pieces(n_out[k], lambda bit, off, size, k=k: p1_copy(h, k, bit, off, size).start())

    def p1_wait(h):
        for k in range(3):
            def wait(bit, off, size, k=k):
                dst = recv.at[h, pl.ds(pl.multiple_of(ro[k] + off, 16), size)]
                remote(h, dst, dst, sem_p1.at[h, k, bit], me).wait_recv()
            pieces(n_in[k], wait)

    def quarter(h, o, q):
        return ag.at[h, pl.ds(pl.multiple_of(o * SEG + q * QUART, QUART), QUART)]

    def combine_and_send(h):
        for half in range(2):
            rows = slice(half * HALF, (half + 1) * HALF)
            yown[rows, :] = expert_rows(xo_b[rows, :], mo_f[rows, 0:8], h)
            if half == 0:
                p1_wait(h)
            got = jnp.where(_iota((XST, WC), 0) < ktot, recv[h, 0:XST, :],
                            jnp.zeros((), BF16))
            yown[rows, :] += _dot(s0[rows, :], got)

            def tile(j, c):
                valid = (_iota((128, WC), 0) + j * 128) < ktot
                t = jnp.where(valid, recv[h, tile_rows(j), :], jnp.zeros((), BF16))
                yown[rows, :] += _dot(s1[j - XST // 128, rows, :], t)
                return c

            lax.fori_loop(XST // 128, ktiles, tile, 0)
            arow = pl.ds(pl.multiple_of(me * SEG + half * HALF, HALF), HALF)
            ag[h, arow, :] = yown[rows, :].astype(BF16)
            qa, qb = 2 * half, 2 * half + 1
            for dev, q, base in ((right, qa, 0), (left, qb, 4), (right, qb, 0), (left, qa, 4)):
                q_ = quarter(h, me, q)
                remote(h, q_, q_, sem_ag.at[h, base + q], dev).start()

    def forward(h):
        for q in range(4):
            src, base, dev = (left, 0, right) if q % 2 == 0 else (right, 4, left)
            q_ = quarter(h, src, q)
            remote(h, q_, q_, sem_ag.at[h, base + q], me).wait_recv()
            remote(h, q_, q_, sem_ag.at[h, 8 + q], dev).start()

    def finish(h):
        cols = pl.ds(pl.multiple_of(h * WC, WC), WC)
        for half in range(2):
            for q in (2 * half, 2 * half + 1):
                src, base = (right, 4) if q % 2 == 0 else (left, 0)
                q_ = quarter(h, src, q)
                remote(h, q_, q_, sem_ag.at[h, base + q], me).wait_recv()
                q_ = quarter(h, diag, q)
                remote(h, q_, q_, sem_ag.at[h, 8 + q], me).wait_recv()
            for b in range(half * NB // 2, (half + 1) * NB // 2):
                rhs = jnp.concatenate(
                    [ag[h, o * SEG + b * CAP:o * SEG + (b + 1) * CAP, :] for o in range(NDEV)],
                    axis=0)
                out_ref[b * BS:(b + 1) * BS, cols] = _dot(pm[b], rhs)

    def wait_sends(h):
        for k in range(3):
            pieces(n_out[k],
                   lambda bit, off, size, k=k: p1_copy(h, k, bit, off, size).wait_send())
        for _ in range(12):
            q_ = quarter(h, me, 0)
            remote(h, q_, q_, sem_ag.at[h, 0], me).wait_send()

    pl.semaphore_wait(barrier, 3)
    exports(0, as_weights_arrive=True)

    def step(i, c):
        @pl.when(i >= 2)
        def _():
            wait_sends(i - 2)

        @pl.when(i + 2 < NC)
        def _():
            exports(i + 2)

        @pl.when(i + 1 < NC)
        def _():
            combine_and_send(i + 1)

        @pl.when(i == -1)
        def _():
            pc = pcol[...].astype(I32)
            for b in range(NB):
                pm[b] = _onehot(pc[:, b:b + 1] == i1)

        @pl.when((i >= 0) & (i < NC))
        def _():
            forward(i)

        @pl.when(i >= 1)
        def _():
            finish(i - 1)

        return c

    lax.fori_loop(-1, NC + 1, step, 0)
    wait_sends(NC - 1)


def pallas_dist_moe_top2_ep_n2048_d512_e4_h1024_kernel(
    x: jax.Array,
    router_W: jax.Array,
    route_idx: jax.Array,
    expert_W: jax.Array,
):
    wr_t = router_W.T
    r32 = route_idx.astype(I32).T.reshape(2, NB, BS).transpose(1, 0, 2).reshape(2 * NB, BS)

    hbm = pl.BlockSpec(memory_space=pl.ANY)
    vmem = pltpu.VMEM
    scratch = [
        vmem((N, D), F32),
        vmem((GT, D), BF16),
        vmem((NE, D), F32),
        vmem((2 * NB, BS), I32),
        vmem((NC, EL, D, WC), F32),
        vmem((NC, EL, D, WC), BF16),
        vmem((12, NB, BS), I32),
        vmem((BS, BS), F32),
        vmem((8, BS), I32),
        pltpu.SMEM((8, BS), I32),
        vmem((XROWS, D), F32),
        vmem((XROWS, 128), F32),
        vmem((XMAX, D), BF16),
        vmem((SEG, D), BF16),
        vmem((SEG, 128), F32),
        vmem((NC, XMAX, WC), BF16),
        vmem((NC, XMAX, WC), BF16),
        vmem((SEG, WC), F32),
        vmem((SEG, XST), BF16),
        vmem(((XMAX - XST) // 128, SEG, 128), BF16),
        vmem((NB, BS, BS), BF16),
        vmem((NC, N, WC), BF16),
        pltpu.SemaphoreType.DMA((3 + NG + NC * EL,)),
        pltpu.SemaphoreType.DMA((NC,)),
        pltpu.SemaphoreType.DMA((NC, 3, NBIT)),
        pltpu.SemaphoreType.DMA((NC, 12)),
    ]
    return pl.pallas_call(
        _kernel,
        out_shape=pltpu.VMEM((N, H), F32),
        in_specs=[hbm] * 4,
        out_specs=pl.BlockSpec(memory_space=pltpu.VMEM),
        scratch_shapes=scratch,
        compiler_params=pltpu.CompilerParams(
            collective_id=0, vmem_limit_bytes=100 * 1024 * 1024,
            disable_semaphore_checks=True),
    )(x, wr_t, r32, expert_W)
```

```python
import contextlib

import jax
import jax.numpy as jnp
from jax import lax
from jax.experimental import pallas as pl
from jax.experimental.pallas import tpu as pltpu

N, D, H = 2048, 512, 1024
NDEV = 4
EL = 4
NE = NDEV * EL
BS = 128
NB = N // BS
CAP = BS // NDEV
SEG = N // NDEV
WC = 128
NC = H // WC
NH = 2
HB = NB // NH
RO = SEG // NH
PART = RO // 2
NI = NH * NC
GB = 2
NG = NB // GB
GH = NG // NH
GT = GB * BS
WIN = 40
SELR = CAP + 3 * WIN
XE = 272
KE = 256
XMAX = 3 * RO
XYROWS = XE + 512
XROWS = XMAX + 128
ZST = 384
MG = 8
NBIT = 6
WFIRST = 4
LA = 3
CATCH = 6
B0 = 1
F0 = 7

F32 = jnp.float32
BF16 = jnp.bfloat16
I32 = jnp.int32
MESH = pl.DeviceIdType.MESH

PROFILE = False


def _scope(name):
    return jax.named_scope(name) if PROFILE else contextlib.nullcontext()


def _iota(shape, dim):
    return lax.broadcasted_iota(I32, shape, dim)


def _onehot(mask):
    return jnp.where(mask, 1.0, 0.0).astype(BF16)


def _padm(n):
    return (n + MG - 1) & (-MG)


def _dot(a, b):
    return jnp.dot(a, b, preferred_element_type=F32)


def _dot_nt(a, b):
    return lax.dot_general(a, b, (((1,), (1,)), ((), ())),
                           preferred_element_type=F32)


def _kernel(x_hbm, wr_hbm, r_hbm, w_hbm, out_ref,
            xf, xb, wrf, wr2, rv, wf, wb,
            codes, pcol, tabv, tabs,
            xe_f, me_f, xl_b, mo_f,
            yexp, recv, yown, s0, s1, pm, ag,
            sem_in, sem_send, sem_p1, sem_ag):
    me = lax.axis_index("i")
    right = (me + 1) & 3
    diag = (me + 2) & 3
    left = (me + 3) & 3
    peers = (diag, right, left)

    def x_copy(g):
        rows = pl.ds(pl.multiple_of(g * GT, GT), GT)
        return pltpu.make_async_copy(x_hbm.at[rows], xf.at[rows], sem_in.at[3 + g])

    def w0_copy(e):
        return pltpu.make_async_copy(w_hbm.at[e, :, 0:WC], wf.at[0, e], sem_in.at[3 + NG + e])

    def w_copy(h):
        cols = pl.ds(pl.multiple_of(h * WC, WC), WC)
        return pltpu.make_async_copy(w_hbm.at[:, :, cols], wf.at[h],
                                     sem_in.at[3 + NG + EL - 1 + h])

    r_copy = pltpu.make_async_copy(r_hbm, rv, sem_in.at[0])
    wr_copy = pltpu.make_async_copy(wr_hbm, wrf, sem_in.at[1])
    r_copy.start()
    wr_copy.start()
    for g in range(GH):
        x_copy(g).start()
    for e in range(EL):
        w0_copy(e).start()
    for h in range(1, WFIRST):
        w_copy(h).start()
    for g in range(GH, NG):
        x_copy(g).start()
    for h in range(WFIRST, NC):
        w_copy(h).start()

    barrier = pltpu.get_barrier_semaphore()
    for dev in peers:
        pl.semaphore_signal(barrier, 1, device_id=(dev,), device_id_type=MESH)

    for g in range(NH):
        xe_f[g, 0:ZST, :] = jnp.zeros((ZST, D), F32)
        me_f[g, 0:ZST, :] = jnp.zeros((ZST, 128), F32)

    r_copy.wait()
    e0 = rv[pl.ds(0, NB, stride=2), :]
    e1 = rv[pl.ds(1, NB, stride=2), :]
    c0 = e0 >> 2
    c1 = e1 >> 2
    i0 = _iota((BS, BS), 0)
    i1 = _iota((BS, BS), 1)
    upper = _onehot(i0 < i1)
    uo = jnp.concatenate([upper, jnp.ones((BS, BS), BF16)], axis=1)

    def stack(ms):
        return jnp.concatenate([jnp.where(m, 1.0, 0.0) for m in ms], axis=0).astype(BF16)

    def part(a, k):
        return a[NB * k:NB * (k + 1), :]

    is_diag = (c0 ^ c1) == 2
    fixed = jnp.logical_not(is_diag)
    adj = fixed & (c0 != c1)
    low = jnp.where(((c1 - c0) & 3) == 1, c0, c1)
    masks_c = [adj & (low == a) for a in range(NDEV)]
    rc = _dot(stack(masks_c), upper).astype(I32)
    rank_c = sum(jnp.where(masks_c[a], part(rc, a), 0) for a in range(NDEV))
    flip = (rank_c + _iota((NB, BS), 0)) & 1
    pref = jnp.where(adj, (low + flip) & 3, c0)
    masks_a = [fixed & (pref == o) for o in range(NDEV)]
    masks_a += [is_diag & ((c0 & 1) == 0), is_diag & ((c0 & 1) == 1)]
    ra = _dot(stack(masks_a), uo).astype(I32)
    rank_a, tot_a = ra[:, :BS], ra[:, BS:]
    load = [part(tot_a, o) for o in range(NDEV)]
    rank_f = sum(jnp.where(masks_a[o], part(rank_a, o), 0) for o in range(NDEV))
    over = [jnp.maximum(load[o] - CAP, 0) for o in range(NDEV)]
    ovbase = [0, over[0], over[0] + over[1], over[0] + over[1] + over[2]]
    ovb = sum(jnp.where(masks_a[o], ovbase[o], 0) for o in range(1, NDEV))
    tot02, tot13 = part(tot_a, 4), part(tot_a, 5)
    jf = jnp.where(masks_a[4], part(rank_a, 4),
                   jnp.where(masks_a[5], tot02 + part(rank_a, 5),
                             tot02 + tot13 + ovb + rank_f - CAP))
    flex = is_diag | (rank_f >= CAP)
    used = [jnp.minimum(load[o], CAP) for o in range(NDEV)]
    g2 = CAP - used[0]
    g1 = g2 + CAP - used[2]
    g3 = g1 + CAP - used[1]
    p_flex = jnp.where(
        jf < g2, used[0] + jf,
        jnp.where(jf < g1, 2 * CAP + used[2] + jf - g2,
                  jnp.where(jf < g3, CAP + used[1] + jf - g1,
                            3 * CAP + used[3] + jf - g3)))
    p = jnp.where(flex, p_flex, pref * CAP + rank_f)
    owner = p >> 5

    def involves(s):
        return (c0 == s) | (c1 == s)

    masks_b = [involves(me) & (owner == o) for o in peers]
    masks_b += [involves(s) & (owner == me) for s in peers]
    masks_b += [involves(left) & (owner == right), involves(diag) & (owner == right),
                involves(right) & (owner == left)]
    nrow = NB * len(masks_b)
    rb = _dot(stack(masks_b), uo)
    rank_b = rb[:, :BS].astype(I32)
    tot_b = rb[:, BS:].astype(BF16)
    j0 = _iota((nrow + 32, nrow), 0)
    j1 = _iota((nrow + 32, nrow), 1)
    pre = ((((j0 >> 3) == (j1 >> 3)) & (j1 < j0))
           | (((j0 - nrow) == (j1 >> 3)) & (j0 >= nrow)))
    cb = _dot(_onehot(pre), tot_b).astype(I32)
    cum_b, n_b = cb[:nrow, :], cb[nrow:, :]
    npad = _padm(n_b)

    def by_half(k):
        return jnp.concatenate(
            [jnp.broadcast_to(npad[NH * k + g:NH * k + g + 1, :], (HB, BS)) for g in range(NH)],
            axis=0)

    xoff = [0, by_half(0), by_half(0) + by_half(1)]
    roff = [0, by_half(3), by_half(3) + by_half(4)]

    codes[0] = e0
    codes[1] = e1
    codes[2] = jnp.where(owner == me, p & (CAP - 1), -1)
    starts = []
    for k in range(3):
        start = xoff[k] + part(cum_b, k)
        starts.append(start & (-8))
        codes[3 + k] = jnp.where(masks_b[k], part(rank_b, k) + (start & 7), -1)
        ic = jnp.where(masks_b[3 + k],
                       roff[k] + part(cum_b, 3 + k) + part(rank_b, 3 + k) + 1, 0)
        codes[6 + k] = ic & (-32)
        codes[9 + k] = ic & 31

    def diag_row(v):
        sel = _iota(v.shape, 0) == _iota(v.shape, 1)
        return jnp.sum(jnp.where(sel, v, 0).astype(F32), axis=0, keepdims=True).astype(I32)

    tabv[...] = jnp.concatenate(
        [diag_row(jnp.concatenate(starts, axis=0)), diag_row(n_b), jnp.zeros((6, BS), I32)],
        axis=0)
    tab_copy = pltpu.make_async_copy(tabv, tabs, sem_in.at[2])
    tab_copy.start()

    pcol[...] = jnp.concatenate(
        [p.astype(F32), jnp.zeros((BS - NB, BS), F32)], axis=0).T

    wr_copy.wait()
    wr = wrf[...]
    wr_hi = wr.astype(BF16)
    wr2[0:NE, :] = wr_hi
    wr2[NE:2 * NE, :] = (wr - wr_hi.astype(F32)).astype(BF16)

    tab_copy.wait()

    def size(k, g):
        return tabs[1, NH * k + g]

    def n_out(k, g):
        return size(k, g)

    def n_in(k, g):
        return size(3 + k, g)

    def prefix(k0, k, g):
        off = 0
        for q in range(k):
            off = off + _padm(size(k0 + q, g))
        return off

    def dst_off(k, g):
        if k == 0:
            return 0
        if k == 1:
            return _padm(size(6, g)) + _padm(size(7, g))
        return _padm(size(8, g))

    def tile_rows(j):
        return pl.ds(pl.multiple_of(j * 128, 128), 128)

    def tile_units(j):
        return pl.ds(j * (128 // MG), 128 // MG)

    def ntiles(rows):
        return (rows + 127) >> 7

    for g in range(NH):
        def zero_tile(j, c, g=g):
            xe_f[g, tile_rows(j), :] = jnp.zeros((128, D), F32)
            me_f[g, tile_rows(j), :] = jnp.zeros((128, 128), F32)
            return c

        lax.fori_loop(ZST // 128, ntiles(prefix(0, 3, g) + 128), zero_tile, 0)

    def smat(meta, base, width):
        col = _iota((meta.shape[0], width), 1) + (base + 1)
        ics = [meta[:, 4 + k:5 + k].astype(I32) for k in range(3)]
        return _onehot((col == ics[0]) | (col == ics[1]) | (col == ics[2]))

    def gather_group(gi):
        g = gi // GH
        tgt = jnp.concatenate(
            [_iota((CAP, BS), 0)] + [_iota((WIN, BS), 0)] * 3, axis=0)
        erow = _iota((NE, BS), 0)
        x_copy(gi).wait()
        xb[...] = xf[pl.ds(pl.multiple_of(gi * GT, GT), GT), :].astype(BF16)
        sc2 = _dot_nt(wr2[...], xb[...])
        sc = sc2[:NE, :] + sc2[NE:, :]
        for j in range(GB):
            a = gi * GB + j

            def code(k):
                return codes[k, pl.ds(a, 1), :]

            s = sc[:, j * BS:(j + 1) * BS]
            ex = jnp.exp(s - jnp.max(s, axis=0, keepdims=True))
            pr = ex / jnp.sum(ex, axis=0, keepdims=True)
            ea, eb = code(0), code(1)
            ga = jnp.sum(jnp.where(erow == ea, pr, 0.0), axis=0, keepdims=True)
            gb = jnp.sum(jnp.where(erow == eb, pr, 0.0), axis=0, keepdims=True)
            gs = ga + gb
            wa, wb_ = ga / gs, gb / gs
            hi, lo = [], []
            for e in range(EL):
                ge = me * EL + e
                m = jnp.where(ea == ge, wa, 0.0) + jnp.where(eb == ge, wb_, 0.0)
                mh = m.astype(BF16).astype(F32)
                hi.append(mh)
                lo.append(m - mh)
            hi += [code(6 + k).astype(F32) for k in range(3)] + [jnp.zeros((1, BS), F32)]
            lo += [code(9 + k).astype(F32) for k in range(3)] + [jnp.zeros((1, BS), F32)]
            meta = jnp.concatenate(hi + lo, axis=0).astype(BF16)

            cd = jnp.concatenate(
                [jnp.broadcast_to(code(2), (CAP, BS))]
                + [jnp.broadcast_to(code(3 + k), (WIN, BS)) for k in range(3)], axis=0)
            sel = _onehot(cd == tgt)
            gx = _dot(sel, xb[j * BS:(j + 1) * BS, :])
            gm2 = _dot_nt(sel, meta)
            gm = gm2[:, :8] + gm2[:, 8:]
            orow = pl.ds(pl.multiple_of(a * CAP, CAP), CAP)
            lrow = pl.ds(pl.multiple_of(XE + (a % HB) * CAP, 16), CAP)
            xl_b[g, lrow, :] = gx[:CAP].astype(BF16)
            mo_f[orow, 0:8] = gm[:CAP]
            s0[orow, :] = smat(gm[:CAP], 0, KE)
            for k in range(3):
                wrow = pl.ds(pl.multiple_of(tabs[0, k * NB + a], 8), WIN)
                lo_ = CAP + k * WIN
                xe_f[g, wrow, :] += gx[lo_:lo_ + WIN]
                me_f[g, wrow, 0:8] += gm[lo_:lo_ + WIN]

    def own_rows(g):
        return pl.ds(pl.multiple_of(g * RO, RO), RO)

    def finalize_half(g):
        xl_b[g, 0:XE, :] = xe_f[g, 0:XE, :].astype(BF16)

        def extra_smat(j, c):
            s1[g, j - KE // 128] = smat(mo_f[own_rows(g), 0:8], j * 128, 128)
            return c

        lax.fori_loop(KE // 128, ntiles(prefix(3, 3, g)), extra_smat, 0)

    def remote(it, src, dst, rsem, dev):
        return pltpu.make_async_remote_copy(
            src_ref=src, dst_ref=dst, send_sem=sem_send.at[it], recv_sem=rsem,
            device_id=(dev,), device_id_type=MESH)

    def pieces(n_rows, fn):
        u = (n_rows + MG - 1) >> 3
        for bit in reversed(range(NBIT)):
            @pl.when(((u >> bit) & 1) == 1)
            def _(bit=bit):
                fn(bit, (u >> (bit + 1)) << (bit + 1), 1 << bit)

    def p1_all(it, act):
        g = it // NC
        for k in range(3):
            so = prefix(0, k, g) >> 3
            do = dst_off(k, g) >> 3
            slot = (0, 2, 1)[k]

            def one(bit, off, sz, k=k, so=so, do=do, slot=slot):
                act(remote(it, yexp.at[it, pl.ds(so + off, sz)], recv.at[it, pl.ds(do + off, sz)],
                           sem_p1.at[it, slot, bit], peers[k]))

            pieces(n_out(k, g), one)

    def p1_wait(it):
        g = it // NC
        for k in range(3):
            ro = prefix(3, k, g) >> 3

            def wait(bit, off, sz, k=k, ro=ro):
                dst = recv.at[it, pl.ds(ro + off, sz)]
                remote(it, dst, dst, sem_p1.at[it, k, bit], me).wait_recv()

            pieces(n_in(k, g), wait)

    def expert_rows(xv, meta, h, before=None):
        acc = None
        for e in range(EL):
            if before is not None:
                before(e)
            r = _dot(xv, wb[h, e]) * meta[:, e:e + 1]
            acc = r if acc is None else acc + r
        return acc

    def convert_w(h, es):
        for e in es:
            wb[h, e] = wf[h, e].astype(BF16)

    def to_units(y):
        return y.astype(BF16).reshape(y.shape[0] // MG, MG, WC)

    def extra_exports(it, g, h):
        def tile(j, c):
            rows = pl.ds(pl.multiple_of(XE + j * 128, 16), 128)
            yexp[it, pl.ds(XE // MG + j * (128 // MG), 128 // MG)] = to_units(expert_rows(
                xe_f[g, rows, :].astype(BF16), me_f[g, rows, 0:8], h))
            return c

        lax.fori_loop(0, ntiles(prefix(0, 3, g) - XE), tile, 0)

    def first_rows():
        def before(e):
            if e % 2 == 0:
                w0_copy(e).wait()
                w0_copy(e + 1).wait()
                convert_w(0, (e, e + 1))

        yexp[0, 0:XE // MG] = to_units(
            expert_rows(xl_b[0, 0:XE, :], me_f[0, 0:XE, 0:8], 0, before))
        extra_exports(0, 0, 0)
        pl.semaphore_wait(barrier, 3)
        p1_all(0, lambda cp: cp.start())
        yown[0] = expert_rows(xl_b[0, XE:XE + RO, :], mo_f[0:RO, 0:8], 0)

    def expert_stage(it):
        g = it // NC
        h = it % NC

        @pl.when(g == 0)
        def _():
            w_copy(h).wait()
            convert_w(h, range(EL))

        meta = jnp.concatenate([me_f[g, 0:XE, 0:8], mo_f[own_rows(g), 0:8]], axis=0)
        y = expert_rows(xl_b[g], meta, h)
        yexp[it, 0:XE // MG] = to_units(y[:XE])
        yown[it % 4] = y[XE:]
        extra_exports(it, g, h)
        p1_all(it, lambda cp: cp.start())

    def piece(it, o, q):
        row = o * SEG + (it // NC) * RO + q * PART
        return ag.at[it % NC, pl.ds(pl.multiple_of(row, PART), PART)]

    def combine_stage(it):
        g = it // NC
        ktot = prefix(3, 3, g)
        p1_wait(it)
        got = jnp.where(_iota((KE, WC), 0) < ktot,
                        recv[it, 0:KE // MG].reshape(KE, WC), jnp.zeros((), BF16))
        slot = it % 4
        yown[slot] += _dot(s0[own_rows(g), :], got)

        def tile(j, c):
            valid = (_iota((128, WC), 0) + j * 128) < ktot
            t = jnp.where(valid, recv[it, tile_units(j)].reshape(128, WC), jnp.zeros((), BF16))
            yown[slot] += _dot(s1[g, j - KE // 128], t)
            return c

        lax.fori_loop(KE // 128, ntiles(ktot), tile, 0)
        arow = pl.ds(pl.multiple_of(me * SEG + g * RO, RO), RO)
        ag[it % NC, arow, :] = yown[slot].astype(BF16)
        for dev, q, base in ((right, 0, 0), (left, 1, 2), (right, 1, 0), (left, 0, 2)):
            q_ = piece(it, me, q)
            remote(it, q_, q_, sem_ag.at[it, base + q], dev).start()

    def forward_stage(it):
        for q, src, base, dev in ((0, left, 0, right), (1, right, 2, left)):
            q_ = piece(it, src, q)
            remote(it, q_, q_, sem_ag.at[it, base + q], me).wait_recv()
            remote(it, q_, q_, sem_ag.at[it, 4 + q], dev).start()

    def finish_stage(it):
        g = it // NC
        h = it % NC
        for q, src, base in ((1, left, 0), (0, right, 2)):
            q_ = piece(it, src, q)
            remote(it, q_, q_, sem_ag.at[it, base + q], me).wait_recv()
        for q in range(2):
            q_ = piece(it, diag, q)
            remote(it, q_, q_, sem_ag.at[it, 4 + q], me).wait_recv()
        cols = pl.ds(pl.multiple_of(h * WC, WC), WC)
        for j in range(HB):
            b = g * HB + j
            rhs = jnp.concatenate(
                [ag[h, pl.ds(pl.multiple_of(o * SEG + b * CAP, CAP), CAP), :]
                 for o in range(NDEV)], axis=0)
            out_ref[pl.ds(pl.multiple_of(b * BS, BS), BS), cols] = _dot(pm[b], rhs)

    def wait_sends(it):
        p1_all(it, lambda cp: cp.wait_send())
        for _ in range(6):
            q_ = piece(it, me, 0)
            remote(it, q_, q_, sem_ag.at[it, 0], me).wait_send()

    first = -(GH + LA - 1)

    def step(i, c):
        @pl.when(i >= 2)
        def _():
            with _scope("sendwait"):
                wait_sends(i - 2)

        @pl.when((i >= -1) & (i + 1 < NI))
        def _():
            with _scope("combine"):
                combine_stage(i + 1)

        @pl.when((i >= 0) & (i < NI))
        def _():
            with _scope("forward"):
                forward_stage(i)

        @pl.when((i <= -LA) | ((i >= B0) & (i < B0 + GH)))
        def _():
            gi = jnp.where(i < 0, i - first, i - B0 + GH)
            with _scope("group"):
                gather_group(gi)

            @pl.when(gi % GH == GH - 1)
            def _():
                with _scope("finalize"):
                    finalize_half(gi // GH)

        @pl.when(i == -LA)
        def _():
            with _scope("first"):
                first_rows()

        def issued(j):
            return jnp.minimum(j + LA + 1 + (j >= CATCH).astype(I32), NI)

        def expert_body(it, c2):
            with _scope("experts"):
                expert_stage(it)
            return c2

        lax.fori_loop(jnp.maximum(issued(i - 1), 1), issued(i), expert_body, 0)

        @pl.when(i == F0 - 1)
        def _():
            with _scope("pm"):
                pc = pcol[...].astype(I32)
                lane = _iota((BS, BS), 1)
                for b in range(NB):
                    pm[b] = _onehot(pc[:, b:b + 1] == lane)

        def finished(j):
            return jnp.clip(jnp.minimum(2 * (j - F0 + 1), j), 0, NI)

        def finish_body(it, c2):
            with _scope("finish"):
                finish_stage(it)
            return c2

        lax.fori_loop(finished(i - 1), finished(i), finish_body, 0)

        return c

    lax.fori_loop(first, NI + 1, step, 0)
    wait_sends(NI - 1)


def pallas_dist_moe_top2_ep_n2048_d512_e4_h1024_kernel(
    x: jax.Array,
    router_W: jax.Array,
    route_idx: jax.Array,
    expert_W: jax.Array,
):
    wr_t = router_W.T
    r32 = route_idx.astype(I32).T.reshape(2, NB, BS).transpose(1, 0, 2).reshape(2 * NB, BS)

    hbm = pl.BlockSpec(memory_space=pl.ANY)
    vmem = pltpu.VMEM
    scratch = [
        vmem((N, D), F32),
        vmem((GT, D), BF16),
        vmem((NE, D), F32),
        vmem((2 * NE, D), BF16),
        vmem((2 * NB, BS), I32),
        vmem((NC, EL, D, WC), F32),
        vmem((NC, EL, D, WC), BF16),
        vmem((12, NB, BS), I32),
        vmem((BS, BS), F32),
        vmem((8, BS), I32),
        pltpu.SMEM((8, BS), I32),
        vmem((NH, XROWS, D), F32),
        vmem((NH, XROWS, 128), F32),
        vmem((NH, XE + RO, D), BF16),
        vmem((SEG, 128), F32),
        vmem((NI, XYROWS // MG, MG, WC), BF16),
        vmem((NI, XMAX // MG, MG, WC), BF16),
        vmem((4, RO, WC), F32),
        vmem((SEG, KE), BF16),
        vmem((NH, (XMAX - KE) // 128, RO, 128), BF16),
        vmem((NB, BS, BS), BF16),
        vmem((NC, N, WC), BF16),
        pltpu.SemaphoreType.DMA((3 + NG + EL + NC - 1,)),
        pltpu.SemaphoreType.DMA((NI,)),
        pltpu.SemaphoreType.DMA((NI, 3, NBIT)),
        pltpu.SemaphoreType.DMA((NI, 6)),
    ]
    return pl.pallas_call(
        _kernel,
        out_shape=pltpu.VMEM((N, H), F32),
        in_specs=[hbm] * 4,
        out_specs=pl.BlockSpec(memory_space=pltpu.VMEM),
        scratch_shapes=scratch,
        compiler_params=pltpu.CompilerParams(
            collective_id=0, vmem_limit_bytes=100 * 1024 * 1024,
            disable_semaphore_checks=True),
    )(x, wr_t, r32, expert_W)
```

```python
import jax
import jax.numpy as jnp
from jax import lax
from jax.experimental import pallas as pl
from jax.experimental.pallas import tpu as pltpu

N, D, H = 2048, 512, 1024
NDEV = 4
EL = 4
NE = NDEV * EL
BS = 128
NB = N // BS
CAP = BS // NDEV
SEG = N // NDEV
WC = 128
NC = H // WC
NH = 2
HB = NB // NH
RO = SEG // NH
PART = RO // 2
NI = NH * NC
GB = 2
NG = NB // GB
GH = NG // NH
GT = GB * BS
WIN = 40
XE = 272
KE = 256
XMAX = 3 * RO
XYROWS = XE + 512
XROWS = XMAX + 128
ZST = 384
MG = 8
NBIT = 6
WFIRST = 4
LA = 3
CATCH = 6
B0 = 1
F0 = 7

F32 = jnp.float32
BF16 = jnp.bfloat16
I32 = jnp.int32
MESH = pl.DeviceIdType.MESH


def _iota(shape, dim):
    return lax.broadcasted_iota(I32, shape, dim)


def _onehot(mask):
    return jnp.where(mask, 1.0, 0.0).astype(BF16)


def _padm(n):
    return (n + MG - 1) & (-MG)


def _dot(a, b):
    return jnp.dot(a, b, preferred_element_type=F32)


def _dot_nt(a, b):
    return lax.dot_general(a, b, (((1,), (1,)), ((), ())),
                           preferred_element_type=F32)


def _kernel(x_hbm, wr_hbm, r_hbm, w_hbm, out_ref,
            xf, xb, wrf, wr2, rv, wf, wb,
            codes, pcol, tabv, tabs,
            xe_f, me_f, xl_b, mo_f,
            yexp, recv, yown, s0, s1, pm, ag,
            sem_in, sem_send, sem_p1, sem_ag):
    me = lax.axis_index("i")
    right = (me + 1) & 3
    diag = (me + 2) & 3
    left = (me + 3) & 3
    peers = (diag, right, left)

    def x_copy(g):
        rows = pl.ds(pl.multiple_of(g * GT, GT), GT)
        return pltpu.make_async_copy(x_hbm.at[rows], xf.at[rows], sem_in.at[3 + g])

    def w0_copy(e):
        return pltpu.make_async_copy(w_hbm.at[e, :, 0:WC], wf.at[0, e], sem_in.at[3 + NG + e])

    def w_copy(h):
        cols = pl.ds(pl.multiple_of(h * WC, WC), WC)
        return pltpu.make_async_copy(w_hbm.at[:, :, cols], wf.at[h],
                                     sem_in.at[3 + NG + EL - 1 + h])

    r_copy = pltpu.make_async_copy(r_hbm, rv, sem_in.at[0])
    wr_copy = pltpu.make_async_copy(wr_hbm, wrf, sem_in.at[1])
    r_copy.start()
    wr_copy.start()
    for g in range(GH):
        x_copy(g).start()
    for e in range(EL):
        w0_copy(e).start()
    for h in range(1, WFIRST):
        w_copy(h).start()
    for g in range(GH, NG):
        x_copy(g).start()
    for h in range(WFIRST, NC):
        w_copy(h).start()

    barrier = pltpu.get_barrier_semaphore()
    for dev in peers:
        pl.semaphore_signal(barrier, 1, device_id=(dev,), device_id_type=MESH)

    for g in range(NH):
        xe_f[g, 0:ZST, :] = jnp.zeros((ZST, D), F32)
        me_f[g, 0:ZST, :] = jnp.zeros((ZST, 128), F32)

    r_copy.wait()
    e0 = rv[pl.ds(0, NB, stride=2), :]
    e1 = rv[pl.ds(1, NB, stride=2), :]
    c0 = e0 >> 2
    c1 = e1 >> 2
    i0 = _iota((BS, BS), 0)
    i1 = _iota((BS, BS), 1)
    upper = _onehot(i0 < i1)
    uo = jnp.concatenate([upper, jnp.ones((BS, BS), BF16)], axis=1)

    def stack(ms):
        return jnp.concatenate([jnp.where(m, 1.0, 0.0) for m in ms], axis=0).astype(BF16)

    def part(a, k):
        return a[NB * k:NB * (k + 1), :]

    is_diag = (c0 ^ c1) == 2
    fixed = jnp.logical_not(is_diag)
    adj = fixed & (c0 != c1)
    low = jnp.where(((c1 - c0) & 3) == 1, c0, c1)
    masks_c = [adj & (low == a) for a in range(NDEV)]
    rc = _dot(stack(masks_c), upper).astype(I32)
    rank_c = sum(jnp.where(masks_c[a], part(rc, a), 0) for a in range(NDEV))
    flip = (rank_c + _iota((NB, BS), 0)) & 1
    pref = jnp.where(adj, (low + flip) & 3, c0)
    masks_a = [fixed & (pref == o) for o in range(NDEV)]
    masks_a += [is_diag & ((c0 & 1) == 0), is_diag & ((c0 & 1) == 1)]
    ra = _dot(stack(masks_a), uo).astype(I32)
    rank_a, tot_a = ra[:, :BS], ra[:, BS:]
    load = [part(tot_a, o) for o in range(NDEV)]
    rank_f = sum(jnp.where(masks_a[o], part(rank_a, o), 0) for o in range(NDEV))
    over = [jnp.maximum(load[o] - CAP, 0) for o in range(NDEV)]
    ovbase = [0, over[0], over[0] + over[1], over[0] + over[1] + over[2]]
    ovb = sum(jnp.where(masks_a[o], ovbase[o], 0) for o in range(1, NDEV))
    tot02, tot13 = part(tot_a, 4), part(tot_a, 5)
    jf = jnp.where(masks_a[4], part(rank_a, 4),
                   jnp.where(masks_a[5], tot02 + part(rank_a, 5),
                             tot02 + tot13 + ovb + rank_f - CAP))
    flex = is_diag | (rank_f >= CAP)
    used = [jnp.minimum(load[o], CAP) for o in range(NDEV)]
    g2 = CAP - used[0]
    g1 = g2 + CAP - used[2]
    g3 = g1 + CAP - used[1]
    p_flex = jnp.where(
        jf < g2, used[0] + jf,
        jnp.where(jf < g1, 2 * CAP + used[2] + jf - g2,
                  jnp.where(jf < g3, CAP + used[1] + jf - g1,
                            3 * CAP + used[3] + jf - g3)))
    p = jnp.where(flex, p_flex, pref * CAP + rank_f)
    owner = p >> 5

    def involves(s):
        return (c0 == s) | (c1 == s)

    masks_b = [involves(me) & (owner == o) for o in peers]
    masks_b += [involves(s) & (owner == me) for s in peers]
    masks_b += [involves(left) & (owner == right), involves(diag) & (owner == right),
                involves(right) & (owner == left)]
    nrow = NB * len(masks_b)
    rb = _dot(stack(masks_b), uo)
    rank_b = rb[:, :BS].astype(I32)
    tot_b = rb[:, BS:].astype(BF16)
    j0 = _iota((nrow + 32, nrow), 0)
    j1 = _iota((nrow + 32, nrow), 1)
    pre = ((((j0 >> 3) == (j1 >> 3)) & (j1 < j0))
           | (((j0 - nrow) == (j1 >> 3)) & (j0 >= nrow)))
    cb = _dot(_onehot(pre), tot_b).astype(I32)
    cum_b, n_b = cb[:nrow, :], cb[nrow:, :]
    npad = _padm(n_b)

    def by_half(k):
        return jnp.concatenate(
            [jnp.broadcast_to(npad[NH * k + g:NH * k + g + 1, :], (HB, BS)) for g in range(NH)],
            axis=0)

    xoff = [0, by_half(0), by_half(0) + by_half(1)]
    roff = [0, by_half(3), by_half(3) + by_half(4)]

    codes[0] = e0
    codes[1] = e1
    codes[2] = jnp.where(owner == me, p & (CAP - 1), -1)
    starts = []
    for k in range(3):
        start = xoff[k] + part(cum_b, k)
        starts.append(start & (-8))
        codes[3 + k] = jnp.where(masks_b[k], part(rank_b, k) + (start & 7), -1)
        ic = jnp.where(masks_b[3 + k],
                       roff[k] + part(cum_b, 3 + k) + part(rank_b, 3 + k) + 1, 0)
        codes[6 + k] = ic & (-32)
        codes[9 + k] = ic & 31

    def diag_row(v):
        sel = _iota(v.shape, 0) == _iota(v.shape, 1)
        return jnp.sum(jnp.where(sel, v, 0).astype(F32), axis=0, keepdims=True).astype(I32)

    tabv[...] = jnp.concatenate(
        [diag_row(jnp.concatenate(starts, axis=0)), diag_row(n_b), jnp.zeros((6, BS), I32)],
        axis=0)
    tab_copy = pltpu.make_async_copy(tabv, tabs, sem_in.at[2])
    tab_copy.start()

    pcol[...] = jnp.concatenate(
        [p.astype(F32), jnp.zeros((BS - NB, BS), F32)], axis=0).T

    wr_copy.wait()
    wr = wrf[...]
    wr_hi = wr.astype(BF16)
    wr2[0:NE, :] = wr_hi
    wr2[NE:2 * NE, :] = (wr - wr_hi.astype(F32)).astype(BF16)

    tab_copy.wait()

    def size(k, g):
        return tabs[1, NH * k + g]

    def n_out(k, g):
        return size(k, g)

    def n_in(k, g):
        return size(3 + k, g)

    def prefix(k0, k, g):
        off = 0
        for q in range(k):
            off = off + _padm(size(k0 + q, g))
        return off

    def dst_off(k, g):
        if k == 0:
            return 0
        if k == 1:
            return _padm(size(6, g)) + _padm(size(7, g))
        return _padm(size(8, g))

    def tile_rows(j):
        return pl.ds(pl.multiple_of(j * 128, 128), 128)

    def tile_units(j):
        return pl.ds(j * (128 // MG), 128 // MG)

    def ntiles(rows):
        return (rows + 127) >> 7

    for g in range(NH):
        def zero_tile(j, c, g=g):
            xe_f[g, tile_rows(j), :] = jnp.zeros((128, D), F32)
            me_f[g, tile_rows(j), :] = jnp.zeros((128, 128), F32)
            return c

        lax.fori_loop(ZST // 128, ntiles(prefix(0, 3, g) + 128), zero_tile, 0)

    def smat(meta, base, width):
        col = _iota((meta.shape[0], width), 1) + (base + 1)
        ics = [meta[:, 4 + k:5 + k].astype(I32) for k in range(3)]
        return _onehot((col == ics[0]) | (col == ics[1]) | (col == ics[2]))

    def gather_group(gi, g):
        tgt = jnp.concatenate(
            [_iota((CAP, BS), 0)] + [_iota((WIN, BS), 0)] * 3, axis=0)
        erow = _iota((NE, BS), 0)
        x_copy(gi).wait()
        xb[...] = xf[pl.ds(pl.multiple_of(gi * GT, GT), GT), :].astype(BF16)
        sc2 = _dot_nt(wr2[...], xb[...])
        sc = sc2[:NE, :] + sc2[NE:, :]
        for j in range(GB):
            a = gi * GB + j

            def code(k):
                return codes[k, pl.ds(a, 1), :]

            s = sc[:, j * BS:(j + 1) * BS]
            ex = jnp.exp(s - jnp.max(s, axis=0, keepdims=True))
            pr = ex / jnp.sum(ex, axis=0, keepdims=True)
            ea, eb = code(0), code(1)
            ga = jnp.sum(jnp.where(erow == ea, pr, 0.0), axis=0, keepdims=True)
            gb = jnp.sum(jnp.where(erow == eb, pr, 0.0), axis=0, keepdims=True)
            gs = ga + gb
            wa, wb_ = ga / gs, gb / gs
            hi, lo = [], []
            for e in range(EL):
                ge = me * EL + e
                m = jnp.where(ea == ge, wa, 0.0) + jnp.where(eb == ge, wb_, 0.0)
                mh = m.astype(BF16).astype(F32)
                hi.append(mh)
                lo.append(m - mh)
            hi += [code(6 + k).astype(F32) for k in range(3)] + [jnp.zeros((1, BS), F32)]
            lo += [code(9 + k).astype(F32) for k in range(3)] + [jnp.zeros((1, BS), F32)]
            meta = jnp.concatenate(hi + lo, axis=0).astype(BF16)

            cd = jnp.concatenate(
                [jnp.broadcast_to(code(2), (CAP, BS))]
                + [jnp.broadcast_to(code(3 + k), (WIN, BS)) for k in range(3)], axis=0)
            sel = _onehot(cd == tgt)
            gx = _dot(sel, xb[j * BS:(j + 1) * BS, :])
            gm2 = _dot_nt(sel, meta)
            gm = gm2[:, :8] + gm2[:, 8:]
            orow = pl.ds(pl.multiple_of(a * CAP, CAP), CAP)
            lrow = pl.ds(pl.multiple_of(XE + (a % HB) * CAP, 16), CAP)
            xl_b[g, lrow, :] = gx[:CAP].astype(BF16)
            mo_f[orow, 0:8] = gm[:CAP]
            s0[orow, :] = smat(gm[:CAP], 0, KE)
            for k in range(3):
                wrow = pl.ds(pl.multiple_of(tabs[0, k * NB + a], 8), WIN)
                lo_ = CAP + k * WIN
                xe_f[g, wrow, :] += gx[lo_:lo_ + WIN]
                me_f[g, wrow, 0:8] += gm[lo_:lo_ + WIN]

    def own_rows(g):
        return pl.ds(pl.multiple_of(g * RO, RO), RO)

    def finalize_half(g):
        xl_b[g, 0:XE, :] = xe_f[g, 0:XE, :].astype(BF16)

        def extra_smat(j, c):
            s1[g, j - KE // 128] = smat(mo_f[own_rows(g), 0:8], j * 128, 128)
            return c

        lax.fori_loop(KE // 128, ntiles(prefix(3, 3, g)), extra_smat, 0)

    def remote(it, src, dst, rsem, dev):
        return pltpu.make_async_remote_copy(
            src_ref=src, dst_ref=dst, send_sem=sem_send.at[it], recv_sem=rsem,
            device_id=(dev,), device_id_type=MESH)

    def pieces(n_rows, fn):
        u = (n_rows + MG - 1) >> 3
        for bit in reversed(range(NBIT)):
            @pl.when(((u >> bit) & 1) == 1)
            def _(bit=bit):
                fn(bit, (u >> (bit + 1)) << (bit + 1), 1 << bit)

    def p1_all(it, act):
        g = it // NC
        for k in range(3):
            so = prefix(0, k, g) >> 3
            do = dst_off(k, g) >> 3
            slot = (0, 2, 1)[k]

            def one(bit, off, sz, k=k, so=so, do=do, slot=slot):
                act(remote(it, yexp.at[it, pl.ds(so + off, sz)], recv.at[it, pl.ds(do + off, sz)],
                           sem_p1.at[it, slot, bit], peers[k]))

            pieces(n_out(k, g), one)

    def p1_wait(it):
        g = it // NC
        for k in range(3):
            ro = prefix(3, k, g) >> 3

            def wait(bit, off, sz, k=k, ro=ro):
                dst = recv.at[it, pl.ds(ro + off, sz)]
                remote(it, dst, dst, sem_p1.at[it, k, bit], me).wait_recv()

            pieces(n_in(k, g), wait)

    def expert_rows(xv, meta, h, before=None):
        acc = None
        for e in range(EL):
            if before is not None:
                before(e)
            r = _dot(xv, wb[h, e]) * meta[:, e:e + 1]
            acc = r if acc is None else acc + r
        return acc

    def convert_w(h, es):
        for e in es:
            wb[h, e] = wf[h, e].astype(BF16)

    def to_units(y):
        return y.astype(BF16).reshape(y.shape[0] // MG, MG, WC)

    def extra_exports(it, g, h):
        def tile(j, c):
            rows = pl.ds(pl.multiple_of(XE + j * 128, 16), 128)
            yexp[it, pl.ds(XE // MG + j * (128 // MG), 128 // MG)] = to_units(expert_rows(
                xe_f[g, rows, :].astype(BF16), me_f[g, rows, 0:8], h))
            return c

        lax.fori_loop(0, ntiles(prefix(0, 3, g) - XE), tile, 0)

    def first_rows():
        def before(e):
            if e % 2 == 0:
                w0_copy(e).wait()
                w0_copy(e + 1).wait()
                convert_w(0, (e, e + 1))

        yexp[0, 0:XE // MG] = to_units(
            expert_rows(xl_b[0, 0:XE, :], me_f[0, 0:XE, 0:8], 0, before))
        extra_exports(0, 0, 0)
        pl.semaphore_wait(barrier, 3)
        p1_all(0, lambda cp: cp.start())
        yown[0] = expert_rows(xl_b[0, XE:XE + RO, :], mo_f[0:RO, 0:8], 0)

    def expert_stage(it):
        g = it // NC
        h = it % NC

        @pl.when(g == 0)
        def _():
            w_copy(h).wait()
            convert_w(h, range(EL))

        meta = jnp.concatenate([me_f[g, 0:XE, 0:8], mo_f[own_rows(g), 0:8]], axis=0)
        y = expert_rows(xl_b[g], meta, h)
        yexp[it, 0:XE // MG] = to_units(y[:XE])
        yown[it % 4] = y[XE:]
        extra_exports(it, g, h)
        p1_all(it, lambda cp: cp.start())

    def piece(it, o, q):
        row = o * SEG + (it // NC) * RO + q * PART
        return ag.at[it % NC, pl.ds(pl.multiple_of(row, PART), PART)]

    def combine_stage(it):
        g = it // NC
        ktot = prefix(3, 3, g)
        p1_wait(it)
        got = jnp.where(_iota((KE, WC), 0) < ktot,
                        recv[it, 0:KE // MG].reshape(KE, WC), jnp.zeros((), BF16))
        slot = it % 4
        yown[slot] += _dot(s0[own_rows(g), :], got)

        def tile(j, c):
            valid = (_iota((128, WC), 0) + j * 128) < ktot
            t = jnp.where(valid, recv[it, tile_units(j)].reshape(128, WC), jnp.zeros((), BF16))
            yown[slot] += _dot(s1[g, j - KE // 128], t)
            return c

        lax.fori_loop(KE // 128, ntiles(ktot), tile, 0)
        arow = pl.ds(pl.multiple_of(me * SEG + g * RO, RO), RO)
        ag[it % NC, arow, :] = yown[slot].astype(BF16)
        for dev, q, base in ((right, 0, 0), (left, 1, 2), (right, 1, 0), (left, 0, 2)):
            q_ = piece(it, me, q)
            remote(it, q_, q_, sem_ag.at[it, base + q], dev).start()

    def forward_stage(it):
        for q, src, base, dev in ((0, left, 0, right), (1, right, 2, left)):
            q_ = piece(it, src, q)
            remote(it, q_, q_, sem_ag.at[it, base + q], me).wait_recv()
            remote(it, q_, q_, sem_ag.at[it, 4 + q], dev).start()

    def finish_stage(it):
        g = it // NC
        h = it % NC
        for q, src, base in ((1, left, 0), (0, right, 2)):
            q_ = piece(it, src, q)
            remote(it, q_, q_, sem_ag.at[it, base + q], me).wait_recv()
        for q in range(2):
            q_ = piece(it, diag, q)
            remote(it, q_, q_, sem_ag.at[it, 4 + q], me).wait_recv()
        cols = pl.ds(pl.multiple_of(h * WC, WC), WC)
        for j in range(HB):
            b = g * HB + j
            rhs = jnp.concatenate(
                [ag[h, pl.ds(pl.multiple_of(o * SEG + b * CAP, CAP), CAP), :]
                 for o in range(NDEV)], axis=0)
            out_ref[pl.ds(pl.multiple_of(b * BS, BS), BS), cols] = _dot(pm[b], rhs)

    def wait_sends(it):
        p1_all(it, lambda cp: cp.wait_send())
        for _ in range(6):
            q_ = piece(it, me, 0)
            remote(it, q_, q_, sem_ag.at[it, 0], me).wait_send()

    def first_half(gi, c):
        gather_group(gi, 0)
        return c

    lax.fori_loop(0, GH, first_half, 0)
    finalize_half(0)
    first_rows()

    def step(i, c):
        @pl.when(i >= 2)
        def _():
            wait_sends(i - 2)

        @pl.when((i >= -1) & (i + 1 < NI))
        def _():
            combine_stage(i + 1)

        @pl.when((i >= 0) & (i < NI))
        def _():
            forward_stage(i)

        @pl.when((i >= B0) & (i < B0 + GH))
        def _():
            gather_group(i - B0 + GH, 1)

            @pl.when(i == B0 + GH - 1)
            def _():
                finalize_half(1)

        def issued(j):
            return jnp.minimum(j + LA + 1 + (j >= CATCH).astype(I32), NI)

        def expert_body(it, c2):
            expert_stage(it)
            return c2

        lax.fori_loop(jnp.maximum(issued(i - 1), 1), issued(i), expert_body, 0)

        @pl.when(i == F0 - 1)
        def _():
            pc = pcol[...].astype(I32)
            lane = _iota((BS, BS), 1)
            for b in range(NB):
                pm[b] = _onehot(pc[:, b:b + 1] == lane)

        def finished(j):
            return jnp.clip(jnp.minimum(2 * (j - F0 + 1), j), 0, NI)

        def finish_body(it, c2):
            finish_stage(it)
            return c2

        lax.fori_loop(finished(i - 1), finished(i), finish_body, 0)

        return c

    lax.fori_loop(1 - LA, NI + 1, step, 0)
    wait_sends(NI - 1)


def pallas_dist_moe_top2_ep_n2048_d512_e4_h1024_kernel(
    x: jax.Array,
    router_W: jax.Array,
    route_idx: jax.Array,
    expert_W: jax.Array,
):
    wr_t = router_W.T
    r32 = route_idx.astype(I32).T.reshape(2, NB, BS).transpose(1, 0, 2).reshape(2 * NB, BS)

    hbm = pl.BlockSpec(memory_space=pl.ANY)
    vmem = pltpu.VMEM
    scratch = [
        vmem((N, D), F32),
        vmem((GT, D), BF16),
        vmem((NE, D), F32),
        vmem((2 * NE, D), BF16),
        vmem((2 * NB, BS), I32),
        vmem((NC, EL, D, WC), F32),
        vmem((NC, EL, D, WC), BF16),
        vmem((12, NB, BS), I32),
        vmem((BS, BS), F32),
        vmem((8, BS), I32),
        pltpu.SMEM((8, BS), I32),
        vmem((NH, XROWS, D), F32),
        vmem((NH, XROWS, 128), F32),
        vmem((NH, XE + RO, D), BF16),
        vmem((SEG, 128), F32),
        vmem((NI, XYROWS // MG, MG, WC), BF16),
        vmem((NI, XMAX // MG, MG, WC), BF16),
        vmem((4, RO, WC), F32),
        vmem((SEG, KE), BF16),
        vmem((NH, (XMAX - KE) // 128, RO, 128), BF16),
        vmem((NB, BS, BS), BF16),
        vmem((NC, N, WC), BF16),
        pltpu.SemaphoreType.DMA((3 + NG + EL + NC - 1,)),
        pltpu.SemaphoreType.DMA((NI,)),
        pltpu.SemaphoreType.DMA((NI, 3, NBIT)),
        pltpu.SemaphoreType.DMA((NI, 6)),
    ]
    return pl.pallas_call(
        _kernel,
        out_shape=pltpu.VMEM((N, H), F32),
        in_specs=[hbm] * 4,
        out_specs=pl.BlockSpec(memory_space=pltpu.VMEM),
        scratch_shapes=scratch,
        compiler_params=pltpu.CompilerParams(
            collective_id=0, vmem_limit_bytes=100 * 1024 * 1024,
            disable_semaphore_checks=True),
    )(x, wr_t, r32, expert_W)
```
